```python
import numpy as np

kernel_name = "dist_rs_then_ag_i_m2048_n1024"

def setup_inputs():
    return {"x": np.random.randn(8192, 1024).astype(np.float32)}

def reference(x: np.ndarray) -> np.ndarray:
    return x.reshape(4, 2048, 1024).sum(axis=0)
```

```python
import functools

import jax
import jax.numpy as jnp
from jax import lax
from jax.experimental import pallas as pl
from jax.experimental.pallas import tpu as pltpu

MESH = pl.DeviceIdType.MESH
BF16, F32 = jnp.bfloat16, jnp.float32
M, N = 2048, 1024
Q = M // 4


def _offsets(sizes):
    out, o = [], 0
    for s in sizes:
        out.append((o, s))
        o += s
    assert o == Q
    return out


def _all_reduce(x, p1=(16, 16, 32, 64, 128, 256), p2=(128, 128, 128, 128), p3=(128, 128, 128, 128), out_dtype=BF16):
    c1, c2, c3 = _offsets(p1), _offsets(p2), _offsets(p3)

    def body(x_hbm, out, xv, s1, r1, part, r2, ld_sem, ldm_sem, ss1, rs1, ss2, rs2, ss3, rs3):
        me = lax.axis_index("i")
        px, py = me ^ 3, me ^ 1
        cx, cy = me >> 1, (me ^ (me >> 1)) & 1
        first, second, coord = (px, py), (py, px), (cx, cy)
        mine = [pl.multiple_of(h * 2 * Q + coord[h] * Q, Q) for h in (0, 1)]
        theirs = [pl.multiple_of(h * 2 * Q + (1 - coord[h]) * Q, Q) for h in (0, 1)]

        def load_theirs(h, i):
            o, n = c1[i]
            return pltpu.make_async_copy(x_hbm.at[pl.ds(theirs[h] + o, n)], xv.at[h, pl.ds(o, n)], ld_sem.at[h * len(c1) + i])

        def load_mine(h):
            return pltpu.make_async_copy(x_hbm.at[pl.ds(mine[h], Q)], xv.at[2 + h], ldm_sem.at[h])

        def rdma(src, dst, ss, rs, k, dev):
            return pltpu.make_async_remote_copy(src, dst, ss.at[k], rs.at[k], device_id=(dev,), device_id_type=MESH)

        def cp1(h, i):
            o, n = c1[i]
            return rdma(s1.at[h, pl.ds(o, n)], r1.at[h, pl.ds(o, n)], ss1, rs1, h * len(c1) + i, first[h])

        def cp2(h, i):
            o, n = c2[i]
            return rdma(part.at[h, pl.ds(o, n)], r2.at[h, pl.ds(o, n)], ss2, rs2, h * len(c2) + i, second[h])

        def cp3(h, i):
            o, n = c3[i]
            rows = out.at[pl.ds(mine[h] + o, n)]
            return rdma(rows, rows, ss3, rs3, h * len(c3) + i, first[h])

        for i in range(len(c1)):
            for h in (0, 1):
                load_theirs(h, i).start()
        bar = pltpu.get_barrier_semaphore()
        for d in (px, py):
            pl.semaphore_signal(bar, inc=1, device_id=(d,), device_id_type=MESH)
        for h in (0, 1):
            load_mine(h).start()

        for i, (o, n) in enumerate(c1):
            for h in (0, 1):
                load_theirs(h, i).wait()
                s1[h, pl.ds(o, n), :] = xv[h, pl.ds(o, n), :].astype(BF16)
                if i == 0 and h == 0:
                    pl.semaphore_wait(bar, 2)
                cp1(h, i).start()
        for h in (0, 1):
            load_mine(h).wait()

        got = [0, 0]
        for i, (o, n) in enumerate(c2):
            for h in (0, 1):
                while got[h] < len(c1) and c1[got[h]][0] < o + n:
                    cp1(h, got[h]).wait_recv()
                    got[h] += 1
                part[h, pl.ds(o, n), :] = (xv[2 + h, pl.ds(o, n), :] + r1[h, pl.ds(o, n), :].astype(F32)).astype(BF16)
                cp2(h, i).start()
        got = [0, 0]
        for i, (o, n) in enumerate(c3):
            for h in (0, 1):
                while got[h] < len(c2) and c2[got[h]][0] < o + n:
                    cp2(h, got[h]).wait_recv()
                    got[h] += 1
                out[pl.ds(mine[h] + o, n), :] = (
                    part[h, pl.ds(o, n), :].astype(F32) + r2[h, pl.ds(o, n), :].astype(F32)).astype(BF16)
                cp3(h, i).start()
        for h in (0, 1):
            for i in range(len(c1)):
                cp1(h, i).wait_send()
            for i in range(len(c2)):
                cp2(h, i).wait_send()
        for i in range(len(c3)):
            for h in (0, 1):
                cp3(h, i).wait()

    dma = pltpu.SemaphoreType.DMA
    out = pl.pallas_call(
        body,
        out_shape=pltpu.VMEM((M, N), BF16),
        in_specs=[pl.BlockSpec(memory_space=pltpu.HBM)],
        out_specs=pl.BlockSpec(memory_space=pltpu.VMEM),
        scratch_shapes=[
            pltpu.VMEM((4, Q, N), F32),
            pltpu.VMEM((2, Q, N), BF16), pltpu.VMEM((2, Q, N), BF16),
            pltpu.VMEM((2, Q, N), BF16), pltpu.VMEM((2, Q, N), BF16),
            dma((2 * len(c1),)), dma((2,)),
            dma((2 * len(c1),)), dma((2 * len(c1),)),
            dma((2 * len(c2),)), dma((2 * len(c2),)),
            dma((2 * len(c3),)), dma((2 * len(c3),)),
        ],
        compiler_params=pltpu.CompilerParams(collective_id=0, vmem_limit_bytes=64 << 20),
    )(x)
    return out.astype(out_dtype)


def pallas_dist_rs_then_ag_i_m2048_n1024_kernel(x: jax.Array):
    return _all_reduce(x)
```

```python
import jax
import jax.numpy as jnp
import numpy as np
from jax import lax
from jax.experimental import pallas as pl
from jax.experimental.pallas import tpu as pltpu

I32, BF16, F32 = jnp.int32, jnp.bfloat16, jnp.float32
M, N = 2048, 1024
QUARTER = M // 4
LANES = 128
GROUP = 32
BLOCK = 8
ROWS = GROUP * BLOCK
BLOCKS = QUARTER // ROWS
STEPS = 3 * BLOCKS
PLANES = 9
DEPTH = 5
HEAD = 2
STACK = HEAD + 3 * BLOCK // 2
PACKET = STACK + PLANES * BLOCK
FIRST = ((7, 8), (6, 7), (4, 6), (0, 4))
LAST = ((0, 7), (7, 8))


def _i32(v):
    v &= 0xFFFFFFFF
    return np.int32(v - (1 << 32) if v >> 31 else v)


def _both(v):
    return _i32(v * 0x00010001)


def _shl(x, n):
    return lax.shift_left(x, jnp.full_like(x, n) if isinstance(n, int) else n)


def _shr(x, n):
    return lax.shift_right_logical(x, jnp.full_like(x, n) if isinstance(n, int) else n)


def _tile(x, j, n=1):
    return x[:, :, LANES * j:LANES * (j + n)]


def _beside(tiles):
    return jnp.concatenate(tiles, axis=2)


def _pick_top(sample):
    a = jnp.abs(sample)
    parts = [_tile(a, j) for j in range(a.shape[2] // LANES)]
    while len(parts) > 1:
        parts = [parts[k] + parts[k + 1] for k in range(0, len(parts), 2)]
    total = jnp.sum(jnp.sum(parts[0], axis=1, keepdims=True), axis=2, keepdims=True)
    top = jnp.broadcast_to(total * (10.8 / (a.shape[1] * a.shape[2])), (a.shape[0], 8, LANES))
    return _shr(pltpu.bitcast(top, I32), 16) & 0x7FFF


def _minuend(top):
    return _beside([top | _shl(top, 16) | _both(0x8000)] * 2)


def _zero_index(top):
    return _beside([jnp.maximum(_shr(top, 8), 6)] * 2)


def _empty_stack(halves):
    zero = jnp.zeros((halves, 8, LANES), I32)
    return [zero] * DEPTH, zero, zero, zero


def _encode_group(words, top, sums, odd, state):
    stack, depth, over, wide = state
    zero = jnp.zeros_like(depth)
    one = _i32(0x80000000)
    minuend = _minuend(top)
    far = _zero_index(top) + 2 if sums else None
    diff = {}
    for half, width in ((1, DEPTH + 1), (0, DEPTH + 1 if odd else DEPTH + 2)):
        high = low = total = None
        for quad in reversed(range(4)):
            j = 8 * half + 2 * quad
            c = minuend - _tile(words[:, 8 * half:8 * half + 8], 2 * quad, 2)
            diff[j], diff[j + 1] = _tile(c, 0), _tile(c, 1)
            q = c & _both(0x7F00)
            length = (_shr(q, 8) + (_shr(q + _both(0x8000 - 0x400), 15) & _both(1))
                      + (_shr(_both(0x80FF) - q, 13) & _both(4)))
            if sums:
                length = length + (_shr(q + _both(0x8000 - 0x600), 15) & _both(1))
            lengths = [length & 0xFFFF, _shr(length, 16)]
            if sums:
                lengths = [jnp.where(n == far, 7, n) for n in lengths]
            bits, used = jnp.full_like(zero, one), None
            for i in reversed(range(4)):
                n = _tile(lengths[i % 2], i // 2)
                bits = _shr(bits, n) | one if i else _shl(_shr(bits, n), 1)
                used = n if used is None else used + n
            wide = wide | used
            if high is None:
                high, total = bits, used
            else:
                carry = _shl(high, 32 - used)
                low = carry if low is None else _shr(low, used) | carry
                high, total = _shr(high, used) | bits, total + used
        whole, k = total >= 32, total & 31
        old = [zero] + stack + [zero] * (width - len(stack))
        t = [jnp.where(whole, old[i], old[i + 1]) for i in range(width)]
        stack = [_shr(t[i], k) | _shl(_shl(t[i - 1], 1), 31 - k) if i else _shr(t[0], k)
                 for i in range(width)]
        stack[0], stack[1] = stack[0] | high, stack[1] | low
        wide = wide | _shr(total, 1)
        depth = depth + total
        over = jnp.maximum(over, depth - 32 * width)
    rest = diff[9] & _both(0x8080)
    for j in range(10, 16):
        rest = _shr(rest, 1) | (diff[j] & _both(0x8080))
    filling = [_shl(diff[9 + j], 8) for j in range(7)] + [_shl(rest, 7), _shr(rest, 1)]
    planes = [(diff[j] & _both(0x80FF)) | (filling[j] & _both(0x7F00)) for j in range(PLANES)]
    pop = 1 if odd else 2
    return planes, stack[:pop], (stack[pop:], jnp.maximum(depth - 32 * pop, 0), over, wide)


def _fixed_bits(planes):
    rest = (_shr(planes[7], 7) & _both(0x00FE)) | (_shl(planes[8], 1) & _both(0xFE00))
    fixed = [p & _both(0x80FF) for p in planes]
    for j in range(7):
        ends = _shl(rest, 6 - j) if j < 6 else rest
        fixed.append((_shr(planes[j], 8) & _both(0x007F)) | (ends & _both(0x8080)))
    return fixed


def _decode_group(popped, top, sums, stack, fixed):
    stack = popped + stack
    zero = jnp.zeros_like(top)
    minuend = _minuend(top)
    far = _zero_index(top) if sums else None
    halves = []
    for half, width in enumerate((DEPTH + 1, DEPTH)):
        high, low, total = stack[0], stack[1], None
        quads = []
        for quad in range(4):
            bits, used, runs = high, 4, []
            for i in range(4):
                run = lax.clz(bits)
                if i < 3:
                    bits = _shl(_shl(bits, 1), run)
                used = run + used
                runs.append(run)
            total = used if total is None else total + used
            if quad < 3:
                high = _shl(high, used) | _shr(low, 32 - used)
                if quad < 2:
                    low = _shl(low, used)
            indices = []
            for run in (_beside(runs[0::2]), _beside(runs[1::2])):
                q = jnp.where(run < 4, (run + 1) & 3, run)
                indices.append(jnp.where(run < 6, q, jnp.where(run == 6, far, run - 1)) if sums else q)
            w = minuend - _shl(indices[0] | _shl(indices[1], 16), 8)
            j = 8 * half + 2 * quad
            quads.append(w - _beside(fixed[j:j + 2]) if fixed else w)
        halves.append(_beside(quads))
        whole, k = total >= 32, total & 31
        old = stack + [zero]
        t = [jnp.where(whole, old[i + 1], old[i]) for i in range(len(stack))]
        stack = [_shl(t[i], k) | _shr(_shr(t[i + 1], 1), 31 - k) if i + 1 < len(t) else _shl(t[i], k)
                 for i in range(width)]
    return jnp.concatenate(halves, axis=1), stack


def _running_sum(count):
    upper = lax.broadcasted_iota(I32, (LANES, LANES), 0) <= lax.broadcasted_iota(I32, (LANES, LANES), 1)
    sums = jnp.dot(count.reshape(-1, LANES).astype(F32).astype(BF16),
                   jnp.where(upper, 1.0, 0.0).astype(BF16), preferred_element_type=F32)
    return sums.astype(I32).reshape(count.shape)


def _at(x, lane):
    return jnp.stack([jnp.take_along_axis(x[h], lane[h], axis=1) for h in range(x.shape[0])])


def _encode_head(top, state):
    stack, depth, over, wide = state
    count = jnp.minimum(_shr(jnp.maximum(depth - 14, 0), 4), 7)
    end = _running_sum(count)
    misfit = (over > 0) | (wide >= 32) | (depth > 29 + 16 * 7) | (end >= 2 * LANES)
    misfit = jnp.max(jnp.max(jnp.where(misfit, 1.0, 0.0), axis=1, keepdims=True), axis=2, keepdims=True)
    misfit = jnp.broadcast_to(misfit, top.shape).astype(I32)
    more = [_shl(stack[k], 29) | _shr(stack[k + 1], 3) for k in range(4)]
    lane = lax.broadcasted_iota(I32, top.shape, 2)
    pivots = [jnp.broadcast_to(end[:, :, k - 1:k], top.shape) for k in range(8, LANES, 8)]
    units = []
    for unit in (lane, lane + LANES):
        base = sum(jnp.where(p <= unit, 8, 0) for p in pivots)
        owner = base + sum(jnp.where(_at(end, base + k) <= unit, 1, 0) for k in range(7))
        j = unit - _at(end - count, owner)
        w = [_at(m, owner) for m in more]
        w = jnp.where(j < 4, jnp.where(j < 2, w[0], w[1]), jnp.where(j < 6, w[2], w[3]))
        units.append(jnp.where((j & 1) == 1, w & 0xFFFF, _shr(w, 16)))
    units[1] = jnp.where(lane == LANES - 1, top | _shl(misfit, 15), units[1])
    return [(stack[0] & -8) | count, units[0] | _shl(units[1], 16)], misfit


def _decode_head(first, pooled):
    header = jnp.broadcast_to(_shr(pooled, 16)[:, :, LANES - 1:], first.shape)
    count = first & 7
    start = _running_sum(count) - count
    units = []
    for j in range(7):
        w = _at(pooled, (start + j) & (LANES - 1))
        units.append(jnp.where(start + j < LANES, w & 0xFFFF, _shr(w, 16)))
    more = [_shl(units[k], 16) | units[k + 1] for k in (0, 2, 4)] + [_shl(units[6], 16)]
    stack = ([(first & -8) | _shr(more[0], 29)]
             + [_shl(more[k], 3) | _shr(more[k + 1], 29) for k in range(3)] + [_shl(more[3], 3)])
    return header & 0x7FFF, _shr(header, 15), stack


def _all_reduce(x_hbm, out, x_vmem, sent, got, spare, tx, rx, load_sem, send_sem, recv_sem, ready):
    me = lax.axis_index("i")
    peer_x, peer_y = me ^ 3, me ^ 1
    at_x, at_y = me >> 1, (me ^ (me >> 1)) & 1
    both = pl.ds(0, 2)

    def pick(h, a, b):
        return (a, b)[h] if isinstance(h, int) else jnp.where(h == 0, a, b)

    def mine(h):
        return QUARTER * (2 * h + pick(h, at_x, at_y))

    def theirs(h):
        return QUARTER * (2 * h + 1 - pick(h, at_x, at_y))

    def span(start, size, unit):
        return pl.ds(start if isinstance(start, int) else pl.multiple_of(start, unit), size)

    def group(g, rows=GROUP // 2):
        return span(g * rows, rows, rows)

    def out_group(quarter, step, g):
        return span(quarter + step % BLOCKS * ROWS + g * GROUP, GROUP, GROUP)


    loads = [(g0 * GROUP, (g1 - g0) * GROUP) for g0, g1 in FIRST] + [(b * ROWS, ROWS) for b in range(1, BLOCKS)]
    loads = [(loads[0][0], 8), (loads[0][0] + 8, loads[0][1] - 8)] + loads[1:]

    def load_theirs(h, i):
        row, rows = loads[i]
        return pltpu.make_async_copy(x_hbm.at[span(theirs(h) + row, rows, 8)], x_vmem.at[0, h, pl.ds(row, rows)],
                                     load_sem.at[2 * (BLOCKS + i) + h])

    def load_mine(h, b):
        return pltpu.make_async_copy(x_hbm.at[span(mine(h) + b * ROWS, ROWS, ROWS)],
                                     x_vmem.at[1, h, pl.ds(b * ROWS, ROWS)], load_sem.at[2 * b + h])

    def remote(src, dst, step, h, k):
        peer = pick(h, peer_y, peer_x) if step // BLOCKS == 1 else pick(h, peer_x, peer_y)
        i = (k * STEPS + step) * 2 + h
        return pltpu.make_async_remote_copy(src, dst, send_sem.at[i], recv_sem.at[i], device_id=(peer,),
                                            device_id_type=pl.DeviceIdType.MESH)

    def cuts(step):
        def planes(ranges):
            return [(STACK + PLANES * g0, PLANES * (g1 - g0)) for g0, g1 in ranges]

        if step == 0:
            return planes(FIRST) + [(0, STACK)]
        return [(0, STACK)] + planes(LAST) if step == STEPS - 1 else [(0, PACKET)]

    def piece(step, h, p):
        vregs = pl.ds(*cuts(step)[p])
        return remote(tx.at[step, h, vregs], rx.at[step, h, vregs], step, h, 1 + p)

    def plain(step, h):
        rows = sent.at[step, h] if step < 2 * BLOCKS else out.at[span(mine(h) + step % BLOCKS * ROWS, ROWS, ROWS)]
        return remote(rows, spare.at[step, h], step, h, 0)


    def values(step, hs, g, rows=GROUP, cols=slice(None)):
        phase, b = divmod(step, BLOCKS)
        x_rows = span(b * ROWS + g * GROUP, rows, GROUP)
        if phase == 0:
            return x_vmem[0, hs, x_rows, cols]
        words = got[step - BLOCKS, hs, span(g * (GROUP // 2), rows // 2, GROUP // 2), cols]
        received = pltpu.bitcast(words, BF16).astype(F32)
        if phase == 1:
            return x_vmem[1, hs, x_rows, cols] + received
        return sent[step - BLOCKS, hs, span(g * GROUP, rows, GROUP), cols].astype(F32) + received

    def sample(step, hs):
        return _beside([values(step, hs, g, 16, pl.ds(g * LANES, LANES)) for g in range(BLOCK)])

    def encode(step, hs, g0, g1, top, state):
        def one(pair, odd, state):
            g = 2 * pair + odd
            v = values(step, hs, g).astype(BF16)
            if step < 2 * BLOCKS:
                sent[step, hs, group(g, GROUP)] = v
                v = sent[step, hs, group(g, GROUP)]
            else:
                rows = [out_group(mine(h), step, g) for h in (0, 1)]
                for h in (0, 1):
                    out[rows[h], :] = v[h]
                v = jnp.stack([out[r, :] for r in rows])
            planes, popped, state = _encode_group(pltpu.bitcast(v, I32), top, step >= BLOCKS, odd, state)
            tx[step, hs, pl.ds(STACK + PLANES * g, PLANES)] = jnp.stack(planes, axis=1)
            tx[step, hs, pl.ds(HEAD + 3 * pair + 2 * odd, len(popped))] = jnp.stack(popped, axis=1)
            return state

        def two(i, state):
            pair = g1 // 2 - 1 - i
            return one(pair, 0, one(pair, 1, state))

        if g1 - g0 == 1:
            return one(g0 // 2, g0 % 2, state)
        return two(0, state) if g1 - g0 == 2 else lax.fori_loop(0, (g1 - g0) // 2, two, state)

    misfits = {}

    def finish(step, order, top, state, first_piece=0):
        head, misfit = _encode_head(top, state)
        for k, h in enumerate(order):
            tx[step, h, pl.ds(0, HEAD)] = jnp.stack([word[k] for word in head])
        for p in range(first_piece, len(cuts(step))):
            for h in order:
                piece(step, h, p).start()
        misfits[step] = [(h, misfit[k, 0, 0]) for k, h in enumerate(order)]
        for h, flag in misfits[step]:
            pl.when(flag != 0)(lambda: plain(step, h).start())

    def wait_sent(step, pieces, with_plain):
        for h, flag in misfits[step]:
            for p in pieces:
                piece(step, h, p).wait_send()
            if with_plain:
                pl.when(flag != 0)(lambda: plain(step, h).wait_send())


    def put(step, hs, g, words):
        if step < 2 * BLOCKS:
            got[step, hs, group(g)] = words
        else:
            for k in range(hs.size):
                out[out_group(theirs(hs.start + k), step, g), :] = pltpu.bitcast(words[k], BF16)

    def fixed_bits(step, g):
        planes = rx[step, both, pl.ds(STACK + PLANES * g, PLANES)]
        return _fixed_bits([planes[:, j] for j in range(PLANES)])

    def decode(step, use, with_planes):
        top, misfit, stack = _decode_head(rx[step, both, 0], rx[step, both, 1])
        flags = [misfit[h, 0, 0] for h in (0, 1)]

        def two(pair, stack):
            popped = rx[step, both, pl.ds(HEAD + 3 * pair, 3)]
            for odd, words in enumerate(([popped[:, 0], popped[:, 1]], [popped[:, 2]])):
                g = 2 * pair + odd
                fixed = fixed_bits(step, g) if with_planes else None
                result, stack = _decode_group(words, top, step >= BLOCKS, stack, fixed)
                use(g, result)
            return stack

        lax.fori_loop(0, BLOCK // 2, two, stack)
        return flags

    def use_plain(step, flags):
        for h in (0, 1):
            @pl.when(flags[h] != 0)
            def _():
                plain(step, h).wait_recv()
                hs = pl.ds(h, 1)
                lax.fori_loop(0, BLOCK, lambda g, _: put(
                    step, hs, g, pltpu.bitcast(spare[step, hs, group(g, GROUP)], I32)), None)

    def receive(step):
        for p in range(len(cuts(step))):
            for h in (0, 1):
                piece(step, h, p).wait_recv()
        use_plain(step, decode(step, lambda g, words: put(step, both, g, words), True))

    def receive_last(step):
        for h in (0, 1):
            piece(step, h, 0).wait_recv()
        flags = decode(step, lambda g, words: put(0, both, g, words), False)

        def one(g, _):
            fixed = fixed_bits(step, g)
            fixed = jnp.concatenate([_beside(fixed[:8]), _beside(fixed[8:])], axis=1)
            put(step, both, g, got[0, both, group(g)] - fixed)

        for p, (g0, g1) in enumerate(LAST):
            wait_sent(step, [p], p == 0)
            for h in (0, 1):
                piece(step, h, 1 + p).wait_recv()
            if g1 - g0 == 1:
                one(g0, None)
            else:
                lax.fori_loop(g0, g1, one, None)
        use_plain(step, flags)
        wait_sent(step, [len(LAST)], False)


    barrier = pltpu.get_barrier_semaphore()
    middle = (me & 1) == 1
    order = [jnp.where(me == 1, 1, 0), jnp.where(me == 1, 0, 1)]

    def signal(sem):
        for peer in (peer_x, peer_y):
            pl.semaphore_signal(sem, inc=1, device_id=(peer,), device_id_type=pl.DeviceIdType.MESH)

    pl.when(me != 2)(lambda: signal(barrier))
    for h in order:
        for i in (0, 1):
            load_theirs(h, i).start()

    @pl.when(me == 2)
    def _():
        pl.semaphore_wait(barrier, 2)
        signal(ready)

    tops, states = [None, None], [_empty_stack(1), _empty_stack(1)]

    def prepare(k, i):
        hs, (g0, g1) = pl.ds(order[k], 1), FIRST[i]
        load_theirs(order[k], i + 1 if i else 0).wait()
        if (k, i) == (0, 0):
            for j in range(2, len(loads)):
                for h in order:
                    load_theirs(h, j).start()
            for b in range(BLOCKS):
                for h in (0, 1):
                    load_mine(h, b).start()
        if i == 0:
            tops[k] = _pick_top(values(0, hs, g0, 8))
            load_theirs(order[k], 1).wait()
        states[k] = encode(0, hs, g0, g1, tops[k], states[k])

    def launch(k, i):
        piece(0, order[k], i).start()

    def joined():
        return jax.tree.map(lambda *xs: jnp.concatenate(xs), *zip(tops, states))

    prepare(0, 0)
    pl.when(middle)(lambda: pl.semaphore_wait(barrier, 1))
    pl.when(me != 0)(lambda: launch(0, 0))
    prepare(1, 0)
    pl.when(me == 2)(lambda: launch(1, 0))
    prepare(0, 1)
    pl.when(me != 0)(lambda: launch(0, 1))

    @pl.when(middle)
    def _():
        pl.semaphore_wait(ready, 1)
        launch(1, 0)

    prepare(1, 1)

    @pl.when(me == 0)
    def _():
        pl.semaphore_wait(barrier, 2)
        launch(0, 0)
        launch(1, 0)
        launch(0, 1)

    launch(1, 1)
    for i in range(2, len(FIRST)):
        for k in (0, 1):
            prepare(k, i)
            launch(k, i)
    finish(0, order, *joined(), len(FIRST))

    for step in range(1, BLOCKS):
        for k in (0, 1):
            hs = pl.ds(order[k], 1)
            load_theirs(order[k], len(FIRST) + step).wait()
            tops[k] = _pick_top(sample(step, hs))
            states[k] = encode(step, hs, 0, BLOCK, tops[k], _empty_stack(1))
        finish(step, order, *joined())

    for step in range(BLOCKS, STEPS):
        receive(step - BLOCKS)
        if step < 2 * BLOCKS:
            for h in (0, 1):
                load_mine(h, step - BLOCKS).wait()
        top = _pick_top(sample(step, both))
        finish(step, (0, 1), top, encode(step, both, 0, BLOCK, top, _empty_stack(2)))

    for step in range(2 * BLOCKS, STEPS - 1):
        receive(step)
    for step in range(STEPS - 1):
        wait_sent(step, range(len(cuts(step))), True)
    receive_last(STEPS - 1)


def pallas_dist_rs_then_ag_i_m2048_n1024_kernel(x: jax.Array):
    packets = pltpu.VMEM((STEPS, 2, PACKET, 8, LANES), I32)
    copies = pltpu.SemaphoreType.DMA(((2 + max(len(FIRST), len(LAST))) * STEPS * 2,))
    return pl.pallas_call(
        _all_reduce,
        out_shape=pltpu.VMEM((M, N), BF16),
        in_specs=[pl.BlockSpec(memory_space=pltpu.HBM)],
        out_specs=pl.BlockSpec(memory_space=pltpu.VMEM),
        scratch_shapes=[
            pltpu.VMEM((2, 2, QUARTER, N), F32),
            pltpu.VMEM((2 * BLOCKS, 2, ROWS, N), BF16),
            pltpu.VMEM((2 * BLOCKS, 2, ROWS // 2, N), I32),
            pltpu.VMEM((STEPS, 2, ROWS, N), BF16),
            packets,
            packets,
            pltpu.SemaphoreType.DMA((2 * (len(FIRST) + 2 * BLOCKS),)),
            copies,
            copies,
            pltpu.SemaphoreType.REGULAR,
        ],
        compiler_params=pltpu.CompilerParams(
            collective_id=0,
            vmem_limit_bytes=64 << 20,
            disable_semaphore_checks=True,
        ),
    )(x)
```
